```python
import numpy as np

kernel_name = "dist_mean_ax0_xy_m1024_n512"

def setup_inputs():
    return {"x": np.random.randn(2048, 1024).astype(np.float32)}

def reference(x: np.ndarray) -> np.ndarray:
    return np.mean(x, axis=0, keepdims=True)
```

```python
import jax
import jax.numpy as jnp
from jax import lax
from jax.experimental import pallas as pl
from jax.experimental.pallas import tpu as pltpu


N_CHUNKS = 8


def pallas_dist_mean_ax0_xy_m1024_n512_kernel(
    x: jax.Array,
):
    m, n = x.shape
    rows = m // N_CHUNKS
    total_rows = 2 * m

    def body(x_hbm, out_ref, xbuf, send_buf, recv_buf, load_sems, send_sem, recv_sem):
        my_x = lax.axis_index("x")
        my_y = lax.axis_index("y")
        nbr = (1 - my_x, my_y)

        copies = []
        for c in range(N_CHUNKS):
            cp = pltpu.make_async_copy(
                x_hbm.at[pl.ds(c * rows, rows)],
                xbuf.at[pl.ds(c * rows, rows)],
                load_sems.at[c],
            )
            cp.start()
            copies.append(cp)

        barrier_sem = pltpu.get_barrier_semaphore()
        pl.semaphore_signal(
            barrier_sem, inc=1, device_id=nbr, device_id_type=pl.DeviceIdType.MESH
        )

        acc = jnp.zeros((8, n), jnp.float32)
        for c in range(N_CHUNKS):
            copies[c].wait()
            blk = xbuf[pl.ds(c * rows, rows), :]
            acc = acc + jnp.sum(blk.reshape(rows // 8, 8, n), axis=0)
        send_buf[...] = jnp.sum(acc, axis=0, keepdims=True)

        pl.semaphore_wait(barrier_sem, 1)
        rdma = pltpu.make_async_remote_copy(
            src_ref=send_buf,
            dst_ref=recv_buf,
            send_sem=send_sem,
            recv_sem=recv_sem,
            device_id=nbr,
            device_id_type=pl.DeviceIdType.MESH,
        )
        rdma.start()
        rdma.wait()
        out_ref[...] = (send_buf[...] + recv_buf[...]) * (1.0 / total_rows)

    return pl.pallas_call(
        body,
        out_shape=jax.ShapeDtypeStruct((1, n), jnp.float32),
        in_specs=[pl.BlockSpec(memory_space=pl.ANY)],
        out_specs=pl.BlockSpec(memory_space=pltpu.VMEM),
        scratch_shapes=[
            pltpu.VMEM((m, n), jnp.float32),
            pltpu.VMEM((1, n), jnp.float32),
            pltpu.VMEM((1, n), jnp.float32),
            pltpu.SemaphoreType.DMA((N_CHUNKS,)),
            pltpu.SemaphoreType.DMA,
            pltpu.SemaphoreType.DMA,
        ],
        compiler_params=pltpu.CompilerParams(collective_id=0),
    )(x)
```

```python
import jax
import jax.numpy as jnp
from jax import lax
from jax.experimental import pallas as pl
from jax.experimental.pallas import tpu as pltpu


def pallas_dist_mean_ax0_xy_m1024_n512_kernel(
    x: jax.Array,
):
    m, n = x.shape
    sizes = [m // 2, 3 * m // 8, m // 8]
    offs = [0, sizes[0], sizes[0] + sizes[1]]
    nch = len(sizes)
    total_rows = 2 * m

    def body(x_hbm, out_ref, xbuf, send_buf, recv_buf, load_sems, send_sem, recv_sem):
        my_x = lax.axis_index("x")
        my_y = lax.axis_index("y")
        nbr = (1 - my_x, my_y)

        copies = []
        for c in range(nch):
            cp = pltpu.make_async_copy(
                x_hbm.at[pl.ds(offs[c], sizes[c])],
                xbuf.at[pl.ds(offs[c], sizes[c])],
                load_sems.at[c],
            )
            cp.start()
            copies.append(cp)

        barrier_sem = pltpu.get_barrier_semaphore()
        pl.semaphore_signal(
            barrier_sem, inc=1, device_id=nbr, device_id_type=pl.DeviceIdType.MESH
        )

        acc = jnp.zeros((8, n), jnp.float32)
        for c in range(nch):
            copies[c].wait()
            blk = xbuf[pl.ds(offs[c], sizes[c]), :]
            acc = acc + jnp.sum(blk.reshape(sizes[c] // 8, 8, n), axis=0)
        send_buf[...] = jnp.sum(acc, axis=0, keepdims=True)

        pl.semaphore_wait(barrier_sem, 1)
        rdma = pltpu.make_async_remote_copy(
            src_ref=send_buf,
            dst_ref=recv_buf,
            send_sem=send_sem,
            recv_sem=recv_sem,
            device_id=nbr,
            device_id_type=pl.DeviceIdType.MESH,
        )
        rdma.start()
        rdma.wait()
        out_ref[...] = (send_buf[...] + recv_buf[...]) * (1.0 / total_rows)

    return pl.pallas_call(
        body,
        out_shape=jax.ShapeDtypeStruct((1, n), jnp.float32),
        in_specs=[pl.BlockSpec(memory_space=pl.ANY)],
        out_specs=pl.BlockSpec(memory_space=pltpu.VMEM),
        scratch_shapes=[
            pltpu.VMEM((m, n), jnp.float32),
            pltpu.VMEM((1, n), jnp.float32),
            pltpu.VMEM((1, n), jnp.float32),
            pltpu.SemaphoreType.DMA((nch,)),
            pltpu.SemaphoreType.DMA,
            pltpu.SemaphoreType.DMA,
        ],
        compiler_params=pltpu.CompilerParams(collective_id=0),
    )(x)
```
